```python
import numpy as np

kernel_name = "dist_sparse_attn_blocksparse_qseq_b2_sq256_skv256_hq4_dh64"

def setup_inputs():
    x = np.random.randn(2, 1024, 512).astype(np.float32)
    Wq = np.random.randn(512, 1024).astype(np.float32) * 0.02
    K_ext = np.random.randn(2, 256, 16, 64).astype(np.float32)
    V_ext = np.random.randn(2, 256, 16, 64).astype(np.float32)
    Wo = np.random.randn(1024, 512).astype(np.float32) * 0.02
    return {"x": x, "Wq": Wq, "K_ext": K_ext, "V_ext": V_ext, "Wo": Wo}

def reference(x, Wq, K_ext, V_ext, Wo):
    B, Sq, Skv, Hq, Dh = 2, 1024, 256, 16, 64
    Q = (x @ Wq).reshape(B, Sq, Hq, Dh)
    qb = (np.arange(Sq) // 64)[:, None]
    kb = (np.arange(Skv) // 64)[None, :]
    mask = (qb == kb) | (kb == 0) | ((qb + kb) % 3 == 0)
    scores = np.einsum('bihd,bjhd->bhij', Q, K_ext).astype(np.float32) * 0.125
    scores = np.where(mask[None, None, :, :], scores, -1e9)
    scores_max = scores.max(axis=-1, keepdims=True)
    w = np.exp(scores - scores_max)
    row_keep = mask.any(axis=1)
    w_sum = np.where(row_keep[None, None, :, None], w.sum(axis=-1, keepdims=True), 1.0)
    w = w / w_sum
    w = np.where(row_keep[None, None, :, None], w, 0.0)
    ctx = np.einsum('bhij,bjhd->bihd', w, V_ext).reshape(B, Sq, Hq * Dh)
    return ctx @ Wo
```

```python
import contextlib

import jax
import jax.numpy as jnp
from jax import lax
from jax.experimental import pallas as pl
from jax.experimental.pallas import tpu as pltpu

N_DEV = 4
B, SQ, D, SKV = 2, 256, 512, 256
T = B * SQ
BLK = 64
MESH = pl.DeviceIdType.MESH
F32, BF16 = jnp.float32, jnp.bfloat16


def make(scopes=False, asym=True, head=64, nochk=True, tailsplit=2):
    def scope(name):
        return jax.named_scope(name) if scopes else contextlib.nullcontext()

    def body(x_hbm, wq_hbm, kt_hbm, vt_hbm, wo_hbm, out,
             x_f, wq_f, wo_f, k_f, v_f, x_b, wq_all, wo_all, ctx,
             ld_sem, send_sem, recv_sem, ready_sem):
        me = lax.axis_index("i")
        left = (me + 3) & 3
        right = (me + 1) & 3
        diag = (me + 2) & 3

        barrier = pltpu.get_barrier_semaphore()

        def signal_nbrs(sem):
            for nbr in (left, right):
                pl.semaphore_signal(sem, inc=1, device_id=(nbr,), device_id_type=MESH)

        n_ld = [0]

        def load(src, dst):
            cp = pltpu.make_async_copy(src, dst, ld_sem.at[n_ld[0]])
            n_ld[0] += 1
            cp.start()
            return cp

        hd, tl = pl.ds(0, head), pl.ds(head, D - head)
        ld_q0 = load(wq_hbm.at[hd], wq_f.at[hd])
        ld_q1 = load(wq_hbm.at[tl], wq_f.at[tl])
        if asym:
            pl.when(me != 2)(lambda: signal_nbrs(barrier))

            @pl.when(me == 2)
            def _():
                pl.semaphore_wait(barrier, 2)
                signal_nbrs(ready_sem)
        else:
            signal_nbrs(barrier)
        ld_x = load(x_hbm, x_f)
        owner = (me, left, right, diag)

        def load_kv(g):
            rows = pl.ds(pl.multiple_of(owner[g] * 256, 256), 256)
            return load(kt_hbm.at[:, rows, :], k_f.at[g]), load(vt_hbm.at[:, rows, :], v_f.at[g])

        kv = [load_kv(0)]
        ld_wo = load(wo_hbm, wo_f)
        kv += [load_kv(g) for g in range(1, 4)]

        def rdma(src, dst, s, r, dev):
            return pltpu.make_async_remote_copy(
                src, dst, send_sem.at[s], recv_sem.at[r], device_id=(dev,), device_id_type=MESH)

        r_qa = rdma(wq_all.at[0], wq_all.at[2], 0, 0, right)
        l_qb = rdma(wq_all.at[1], wq_all.at[5], 1, 1, left)
        r_qa0 = rdma(wq_all.at[0, hd], wq_all.at[2, hd], 0, 0, right)
        r_qa1 = rdma(wq_all.at[0, tl], wq_all.at[2, tl], 0, 0, right)
        l_qb0 = rdma(wq_all.at[1, hd], wq_all.at[5, hd], 1, 1, left)
        l_qb1 = rdma(wq_all.at[1, tl], wq_all.at[5, tl], 1, 1, left)
        r_qb = rdma(wq_all.at[1], wq_all.at[3], 2, 2, right)
        l_qa = rdma(wq_all.at[0], wq_all.at[4], 3, 3, left)
        r_fq = rdma(wq_all.at[2], wq_all.at[6], 4, 4, right)
        l_fq = rdma(wq_all.at[5], wq_all.at[7], 5, 5, left)
        r_oa = rdma(wo_all.at[0], wo_all.at[2], 6, 6, right)
        l_ob = rdma(wo_all.at[1], wo_all.at[5], 7, 7, left)
        r_ob = rdma(wo_all.at[1], wo_all.at[3], 8, 8, right)
        l_oa = rdma(wo_all.at[0], wo_all.at[4], 9, 9, left)
        r_f0 = rdma(wo_all.at[2, pl.ds(0, 3)], wo_all.at[6, pl.ds(0, 3)], 10, 10, right)
        l_f0 = rdma(wo_all.at[5, pl.ds(0, 3)], wo_all.at[7, pl.ds(0, 3)], 11, 11, left)
        r_f1 = rdma(wo_all.at[2, 3], wo_all.at[6, 3], 12, 12, right)
        l_f1 = rdma(wo_all.at[5, 3], wo_all.at[7, 3], 13, 13, left)

        def cast_wq(rows):
            for p in range(2):
                wq_all[p, rows, :] = wq_f[rows, p * 128:(p + 1) * 128].astype(BF16)

        with scope("ld_q0"):
            ld_q0.wait()
        cast_wq(hd)
        if asym:
            @pl.when(me == 1)
            def _():
                pl.semaphore_wait(barrier, 1)
                l_qb0.start()

            @pl.when(me == 3)
            def _():
                pl.semaphore_wait(barrier, 1)
                r_qa0.start()
        with scope("ld_q1"):
            ld_q1.wait()
        cast_wq(tl)
        with scope("start_q"):
            if asym:
                @pl.when(me == 1)
                def _():
                    l_qb1.start()
                    l_qa.start()
                    pl.semaphore_wait(ready_sem, 1)
                    r_qa.start()
                    r_qb.start()

                @pl.when(me == 3)
                def _():
                    r_qa1.start()
                    r_qb.start()
                    pl.semaphore_wait(ready_sem, 1)
                    l_qb.start()
                    l_qa.start()

                @pl.when((me & 1) == 0)
                def _():
                    pl.when(me == 0)(lambda: pl.semaphore_wait(barrier, 2))
                    for cp in (r_qa, l_qb, r_qb, l_qa):
                        cp.start()
            else:
                pl.semaphore_wait(barrier, 2)
                for cp in (r_qa0, l_qb0, r_qa1, l_qb1, r_qb, l_qa):
                    cp.start()

        with scope("ld_x"):
            ld_x.wait()
        x_b[...] = x_f[...].astype(BF16)

        row = lax.broadcasted_iota(jnp.int32, (SQ, SKV), 0)
        col = lax.broadcasted_iota(jnp.int32, (SQ, SKV), 1)
        qb = me * (SQ // BLK) + row // BLK
        kb = col // BLK
        mask = (qb == kb) | (kb == 0) | (lax.rem(qb + kb, 3) == 0)
        low = lax.broadcasted_iota(jnp.int32, (SQ, 128), 1) < 64

        def attend(slot):
            g, p = slot // 2, slot % 2
            q = jnp.dot(x_b[...], wq_all[slot], preferred_element_type=F32) * 0.125
            for b in range(B):
                qb_ = q[b * SQ:(b + 1) * SQ]
                kt = k_f[g, b, p * 128:(p + 1) * 128, :].astype(BF16)
                vt = v_f[g, b, p * 128:(p + 1) * 128, :].astype(BF16)
                lhs = jnp.concatenate(
                    [jnp.where(low, qb_, 0.0), jnp.where(low, 0.0, qb_)], axis=0).astype(BF16)
                s = jnp.dot(lhs, kt, preferred_element_type=F32)
                ps, ls = [], []
                for h in range(2):
                    sh = jnp.where(mask, s[h * SQ:(h + 1) * SQ], -1e9)
                    m = jnp.max(sh, axis=-1, keepdims=True)
                    e = jnp.exp(sh - m)
                    ls.append(jnp.sum(e, axis=-1, keepdims=True))
                    ps.append(e.astype(BF16))
                o = lax.dot_general(jnp.concatenate(ps, axis=0), vt, (((1,), (1,)), ((), ())),
                                    preferred_element_type=F32)
                c = jnp.where(low, o[:SQ], o[SQ:]) / jnp.where(low, ls[0], ls[1])
                ctx[slot, b * SQ:(b + 1) * SQ, :] = c.astype(BF16)

        def oproj(slots, cols, first=False, split=1):
            for h in range(split):
                rows = pl.ds(h * (T // split), T // split)
                lhs = jnp.concatenate([ctx[s, rows, :] for s in slots], axis=1)
                for c in cols:
                    rhs = jnp.concatenate([wo_all[s, c] for s in slots], axis=0)
                    o = jnp.dot(lhs, rhs, preferred_element_type=F32)
                    if first:
                        out[rows, c * 128:(c + 1) * 128] = o
                    else:
                        out[rows, c * 128:(c + 1) * 128] += o

        with scope("ld_kv0"):
            kv[0][0].wait()
            kv[0][1].wait()
        with scope("attn01"):
            attend(0)
            attend(1)
        with scope("ld_wo"):
            ld_wo.wait()
        for p in range(2):
            for c in range(4):
                wo_all[p, c] = wo_f[p * 128:(p + 1) * 128, c * 128:(c + 1) * 128].astype(BF16)

        with scope("w_q1"):
            r_qa.wait_recv()
            l_qb.wait_recv()
        for cp in (r_fq, l_fq, r_oa, l_ob, r_ob, l_oa):
            cp.start()
        for g in (1, 2):
            kv[g][0].wait()
            kv[g][1].wait()
        with scope("attn25"):
            attend(2)
            attend(5)
        with scope("w_q2"):
            r_qb.wait_recv()
            l_qa.wait_recv()
        with scope("attn34"):
            attend(3)
            attend(4)
        with scope("w_q3"):
            r_fq.wait_recv()
            l_fq.wait_recv()
        kv[3][0].wait()
        kv[3][1].wait()
        with scope("attn67"):
            attend(6)
            attend(7)
        with scope("w_o1"):
            r_oa.wait_recv()
            l_ob.wait_recv()
        for cp in (r_f0, l_f0, r_f1, l_f1):
            cp.start()
        with scope("op1"):
            oproj((0, 1, 2, 5), range(4), first=True)
        with scope("w_o2"):
            r_ob.wait_recv()
            l_oa.wait_recv()
        with scope("op2"):
            oproj((3, 4), range(4))
        with scope("w_send"):
            for cp in (r_qa, l_qb, r_qb, l_qa, r_fq, l_fq, r_oa, l_ob, r_ob, l_oa):
                cp.wait_send()
        with scope("w_o3"):
            r_f0.wait_recv()
            l_f0.wait_recv()
        with scope("op3"):
            oproj((6, 7), range(3), split=tailsplit)
        with scope("w_o4"):
            r_f1.wait_recv()
            l_f1.wait_recv()
        with scope("op4"):
            oproj((6, 7), (3,), split=tailsplit)
        with scope("w_send2"):
            for cp in (r_f0, l_f0, r_f1, l_f1):
                cp.wait_send()

    def fn(x, Wq, K_ext, V_ext, Wo):
        kt = jnp.transpose(K_ext, (0, 2, 3, 1)).reshape(B, 1024, SKV)
        vt = jnp.transpose(V_ext, (0, 2, 3, 1)).reshape(B, 1024, SKV)
        hbm = pl.BlockSpec(memory_space=pltpu.HBM)
        out = pl.pallas_call(
            body,
            out_shape=pltpu.VMEM((T, D), F32),
            in_specs=[hbm] * 5,
            out_specs=pl.BlockSpec(memory_space=pltpu.VMEM),
            scratch_shapes=[
                pltpu.VMEM((T, D), F32),
                pltpu.VMEM((D, 256), F32),
                pltpu.VMEM((256, D), F32),
                pltpu.VMEM((4, B, 256, SKV), F32),
                pltpu.VMEM((4, B, 256, SKV), F32),
                pltpu.VMEM((T, D), BF16),
                pltpu.VMEM((8, D, 128), BF16),
                pltpu.VMEM((8, 4, 128, 128), BF16),
                pltpu.VMEM((8, T, 128), BF16),
                pltpu.SemaphoreType.DMA((12,)),
                pltpu.SemaphoreType.DMA((14,)),
                pltpu.SemaphoreType.DMA((14,)),
                pltpu.SemaphoreType.REGULAR,
            ],
            compiler_params=pltpu.CompilerParams(
                collective_id=0, vmem_limit_bytes=48 * 2**20,
                disable_bounds_checks=nochk, disable_semaphore_checks=nochk),
        )(x.reshape(T, D), Wq, kt, vt, Wo)
        return out.reshape(B, SQ, D)

    return fn


def pallas_dist_sparse_attn_blocksparse_qseq_b2_sq256_skv256_hq4_dh64_kernel(x, Wq, K_ext, V_ext, Wo):
    return make()(x, Wq, K_ext, V_ext, Wo)
```

```python
import functools
import math

import jax
import jax.numpy as jnp
from jax import lax
from jax.experimental import pallas as pl
from jax.experimental.pallas import tpu as pltpu

B, SQ, D, SKV = 2, 256, 512, 256
T = B * SQ
BLK = 64
F32, BF16, I32 = jnp.float32, jnp.bfloat16, jnp.int32
OUT_DTYPE = BF16
MESH = pl.DeviceIdType.MESH
Q_SCALE = 0.125 * math.log2(math.e)
WQ, WO = 0, 1
FIRST_SPANS = ((0, 64), (64, 192), (192, D))

WORDS, CODES = 256, 192
MAX_FIXES = 3


def _s32(v):
    return v - (1 << 32) if v >= 1 << 31 else v


SIGN_MANT, SIGNS = _s32(0x807F807F), _s32(0x80008000)
EXP_LOW, EXP_HIGH = 0x07800780, 0x78007800
_srl = lax.shift_right_logical


def _vregs(x):
    return [x[i:i + 8] for i in range(0, x.shape[0], 8)]


def _lane_max(vregs):
    top = jnp.max(functools.reduce(jnp.maximum, vregs), axis=0, keepdims=True)
    return jnp.broadcast_to(top, (8, 128))


def _words(x):
    return pltpu.bitcast(x.astype(BF16), I32)


def _choose_base(x, margin):
    top = _srl(pltpu.bitcast(_lane_max(_vregs(jnp.abs(x))), I32), 23)
    return jnp.clip(top + (margin - 15), 0, 240)


def _both_halves(base):
    return (base << 7) | (base << 23)


def _drop_high_exp(word, shift):
    return (word & SIGN_MANT) | (((word | SIGNS) - shift) & EXP_LOW)


def _encode(words, base):
    c = [_drop_high_exp(w, _both_halves(base)) for w in _vregs(words)]
    out = []
    for i in range(0, len(c), 4):
        d = c[i + 3]
        out += [
            c[i] | ((d << 11) & EXP_HIGH),
            c[i + 1] | ((d << 7) & EXP_HIGH),
            c[i + 2] | ((d << 3) & 0x38003800) | (_srl(d, 1) & 0x40004000),
        ]
    return jnp.concatenate(out, axis=0)


def _decode(codes, base):
    shift = _both_halves(base)
    v = _vregs(codes)
    out = []
    for i in range(0, len(v), 3):
        a, b, c = v[i:i + 3]
        d = (_srl(a & EXP_HIGH, 11) | _srl(b & EXP_HIGH, 7)) | (
            _srl(c & 0x38003800, 3) | ((c & 0x40004000) << 1))
        out += [(x & ~EXP_HIGH) + shift for x in (a, b, c)] + [d + shift]
    return out


def _misfits(words, base):
    shift = _both_halves(base)
    row = lax.broadcasted_iota(I32, (8, 128), 0)
    keys = []
    for i, w in enumerate(_vregs(words)):
        flip = (_drop_high_exp(w, shift) + shift) ^ w
        keys.append(jnp.where(flip != 0, flip | (row + 8 * i), 0))
    return keys


def _pack_fix(key):
    return (key & 0xFF) | ((key >> 3) & 0x0F00) | ((key >> 15) & 0xF000)


def _read_header(h0, h1):
    row = lax.broadcasted_iota(I32, (8, 128), 0)
    fixes = [(jnp.where((f & 7) == row, (f >> 3) & 31, -1), ((f & 0x0F00) << 3) | ((f & 0xF000) << 15))
             for f in (h1 & 0xFFFF, _srl(h0, 16), h0 & 0xFFFF)]
    flips = []
    for i in range(WORDS // 8):
        flip = 0
        for vreg, bits in fixes:
            flip = jnp.where(vreg == i, bits, flip)
        flips.append(flip)
    return (h1 >> 16) & 0xFF, flips


def _first_head(rows):
    return lax.broadcasted_iota(I32, (rows, 128), 1) < BLK


def _nn(a, b):
    return jnp.dot(a, b, preferred_element_type=F32)


def _nt(a, b):
    return lax.dot_general(a, b, (((1,), (1,)), ((), ())), preferred_element_type=F32)


def _stack_heads(q):
    first = _first_head(q.shape[0])
    return jnp.concatenate([jnp.where(first, q, 0.0), jnp.where(first, 0.0, q)], axis=0).astype(BF16)


def _exp_and_sums(s, mask=None):
    n = s.shape[0] // 2
    es, sums = [], []
    for h in range(2):
        sh = s[h * n:(h + 1) * n]
        if mask is not None:
            sh = jnp.where(mask, sh, -1e9)
        e = jnp.exp2(sh - jnp.max(sh, axis=-1, keepdims=True))
        es.append(e)
        sums.append(jnp.sum(e, axis=-1, keepdims=True))
    return jnp.concatenate(es, axis=0).astype(BF16), sums


def _normalize(o, sums):
    n = o.shape[0] // 2
    first = _first_head(n)
    total = jnp.where(first, sums[0], sums[1])
    r = pl.reciprocal(total, approx=True)
    r = r * (2.0 - total * r)
    return (jnp.where(first, o[:n], o[n:]) * r).astype(BF16)


def _kernel_body(x_hbm, wq_hbm, kt_hbm, vt_hbm, wo_hbm, out,
                 x_f, wq_f, wo_f, k_f, v_f, x_b, q_own, words, codes, heads, ctx, mixed, acc,
                 load_sem, send_sem, recv_sem, ready_sem):
    me = lax.axis_index("i")
    left, right, diag = (me + 3) & 3, (me + 1) & 3, (me + 2) & 3
    owner = (me, left, right, diag)

    loads = []

    def load(src, dst):
        loads.append(pltpu.make_async_copy(src, dst, load_sem.at[len(loads)]))
        loads[-1].start()
        return loads[-1]

    lead = (me == 1).astype(I32)
    pair = (lead, 1 - lead)
    load_wq = [[load(wq_hbm.at[pl.ds(a, b - a), pl.ds(pl.multiple_of(pair[j] * 128, 128), 128)],
                     wq_f.at[j, pl.ds(a, b - a)]) for j in range(2)] for a, b in FIRST_SPANS]

    barrier = pltpu.get_barrier_semaphore()

    def signal_neighbours(sem):
        for chip in (left, right):
            pl.semaphore_signal(sem, inc=1, device_id=(chip,), device_id_type=MESH)

    pl.when(me != 2)(lambda: signal_neighbours(barrier))

    @pl.when(me == 2)
    def _():
        pl.semaphore_wait(barrier, 2)
        signal_neighbours(ready_sem)

    def load_kv(slot):
        rows = pl.ds(pl.multiple_of(owner[slot // 2] * 256 + (slot % 2) * 128, 128), 128)
        return [load(src.at[:, rows, :], dst.at[slot]) for src, dst in ((kt_hbm, k_f), (vt_hbm, v_f))]

    load_x = load(x_hbm, x_f)
    load_wo = load(wo_hbm, wo_f)
    load_kvs = {slot: load_kv(slot) for slot in (0, 1, 2, 5, 3, 4, 6, 7)}

    plain = {}
    hops, recv_sems = [], []

    class Hop:
        def __init__(self, m, src, dst, chip, send_in=(), arrive_in=((0, CODES),)):
            def copy(ref, span, sent, received):
                rows = pl.ds(span[0], span[1] - span[0])
                return pltpu.make_async_remote_copy(
                    ref.at[m, src, rows], ref.at[m, dst, rows], send_sem.at[sent], received,
                    device_id=(chip,), device_id_type=MESH)

            def new_sem():
                recv_sems.append(recv_sem.at[len(recv_sems)])
                return recv_sems[-1]

            self.src, self.dst = (m, src), (m, dst)
            self.codes = [copy(codes, span, 0, new_sem()) for span in arrive_in]
            self.parts = [copy(codes, span, 0, recv_sems[-1]) for span in send_in]
            self.head = copy(heads, (0, 2), 1, new_sem())
            self.words = copy(words, (0, WORDS), 2 + len(hops), new_sem())
            hops.append(self)

        def start(self, with_codes=True):
            self.head.start()
            if with_codes:
                for cp in self.codes:
                    cp.start()
            pl.when(plain[self.src])(self.words.start)

    parts = tuple((a * 3 // 8, b * 3 // 8) for a, b in FIRST_SPANS)
    tail = ((0, 96), (96, 144))
    q_first = Hop(WQ, 0, 2, right, parts), Hop(WQ, 1, 5, left, parts)
    q_second = Hop(WQ, 1, 3, right), Hop(WQ, 0, 4, left)
    o_first = Hop(WO, 0, 2, right), Hop(WO, 1, 5, left)
    q_far = Hop(WQ, 2, 6, right), Hop(WQ, 5, 7, left)
    o_second = Hop(WO, 1, 3, right), Hop(WO, 0, 4, left)
    o_far = (Hop(WO, 2, 6, right, (), (*tail, (144, 168), (168, CODES))),
             Hop(WO, 5, 7, left, (), (*tail, (168, CODES), (144, 168))))

    def write_headers(m, slots, bases):
        counts = []
        for slot, base in zip(slots, bases):
            keys = _misfits(words[m, slot], base)
            n = functools.reduce(jnp.add, [jnp.where(k != 0, 1.0, 0.0) for k in keys])
            n = jnp.max(jnp.sum(n, axis=0, keepdims=True), axis=1, keepdims=True)
            n = jnp.broadcast_to(n, (8, 128)).astype(I32)
            h1 = (base << 16) | jnp.where(n > MAX_FIXES, 1 << 24, 0)
            row = lax.broadcasted_iota(I32, (8, 128), 0)
            heads[m, slot] = jnp.where(row == 0, _pack_fix(_lane_max(keys)), h1)[:2]
            counts.append(n)
        both = (counts[0] | (counts[1] << 16))[0, 0]
        counts = (both & 0xFFFF, both >> 16)
        for slot, base, n in zip(slots, bases, counts):
            @pl.when(n > 1)
            def _():
                keys = _misfits(words[m, slot], base)
                found = [_lane_max(keys)]
                for _ in range(2):
                    found.append(_lane_max([jnp.where(k < found[-1], k, 0) for k in keys]))
                row = lax.broadcasted_iota(I32, (8, 128), 0)
                heads[m, slot] |= jnp.where(row == 0, _pack_fix(found[1]) << 16, _pack_fix(found[2]))[:2]
        return [n > MAX_FIXES for n in counts]

    def receive_headers(hop_pair):
        a, b = hop_pair
        a.head.wait_recv()
        b.head.wait_recv()
        both = ((heads[a.dst] >> 24) | (heads[b.dst] >> 24 << 1))[1, 0]
        plain[a.dst], plain[b.dst] = (both & 1) == 1, both > 1

    def receive(hop_pair, i=0):
        for hop in hop_pair:
            hop.codes[i].wait_recv()
        if i == 0:
            for hop in hop_pair:
                pl.when(plain[hop.dst])(hop.words.wait_recv)

    def read_header(m, slot):
        return _read_header(*(jnp.broadcast_to(heads[m, slot, k:k + 1, :], (8, 128)) for k in range(2)))

    def weights(m, slot, lo=0, hi=WORDS, header=None):
        if slot < 2:
            return words[m, slot, pl.ds(lo, hi - lo), :]
        base, flips = header or read_header(m, slot)
        decoded = _decode(codes[m, slot, pl.ds(lo * 3 // 4, (hi - lo) * 3 // 4), :], base)
        decoded = jnp.concatenate([w ^ f for w, f in zip(decoded, flips[lo // 8:])], axis=0)
        sent_plain = words[m, jnp.where(plain[m, slot], slot, 0), pl.ds(lo, hi - lo), :]
        return jnp.where(plain[m, slot], sent_plain, decoded)

    bases = [None, None]
    for i, (a, b) in enumerate(FIRST_SPANS):
        for j in range(2):
            load_wq[i][j].wait()
            w = wq_f[j, a:b, :]
            if i == 0:
                bases[j] = _choose_base(w, 1)
            w = _words(w)
            codes[WQ, pair[j], pl.ds(a * 3 // 8, (b - a) * 3 // 8), :] = _encode(w, bases[j])
            if j == 0:
                if i == 0:
                    pl.when((me & 1) == 1)(lambda: pl.semaphore_wait(barrier, 1))
                pl.when(me == 1)(q_first[1].parts[i].start)
                pl.when(me >= 2)(q_first[0].parts[i].start)
            else:
                pl.when(me == 2)(q_first[1].parts[i].start)
            words[WQ, pair[j], pl.ds(a // 2, (b - a) // 2), :] = w

    lead_plain, other_plain = write_headers(WQ, pair, bases)
    plain[WQ, 0] = jnp.where(lead == 0, lead_plain, other_plain)
    plain[WQ, 1] = jnp.where(lead == 0, other_plain, lead_plain)

    for chip, near, far in ((1, 1, 0), (3, 0, 1)):
        @pl.when(me == chip)
        def _():
            q_first[near].start(with_codes=False)
            q_second[near].start()
            pl.semaphore_wait(ready_sem, 1)
            q_first[far].start()
            q_second[far].start()

    @pl.when(me == 0)
    def _():
        pl.semaphore_wait(barrier, 2)
        for hop in (*q_first, *q_second):
            hop.start()

    @pl.when(me == 2)
    def _():
        for hop in q_first:
            hop.start(with_codes=False)
        for hop in q_second:
            hop.start()

    qb0 = me * (SQ // BLK)
    kb = 3 - lax.rem(qb0, 3)
    col = lax.broadcasted_iota(I32, (BLK, SKV), 1) // BLK
    mask = jnp.concatenate(
        [(col == qb0 + i) | (col == 0) | (col == 3 - lax.rem(qb0 + i, 3)) for i in (1, 2)], axis=0)

    def two_blocks(ref, slot, b):
        tile = ref[slot, b, :, pl.ds(pl.multiple_of((kb >> 1) * 128, 128), 128)]
        tile = pltpu.roll(tile, (1 - (kb & 1)) * BLK, 1)
        return jnp.where(_first_head(128), ref[slot, b, :, 0:128], tile).astype(BF16)

    def project(w):
        return _nn(x_b[...], pltpu.bitcast(w, BF16)) * Q_SCALE

    def scores(slot, q, b):
        o = b * SQ
        outer = jnp.concatenate([q[o:o + BLK], q[o + 3 * BLK:o + SQ]], axis=0)
        return (_nn(_stack_heads(q[o + BLK:o + 3 * BLK]), k_f[slot, b].astype(BF16)),
                _nn(_stack_heads(outer), two_blocks(k_f, slot, b)))

    def context(slot, s, b):
        o = b * SQ
        (e1, l1), (e0, l0) = _exp_and_sums(s[0], mask), _exp_and_sums(s[1])
        ctx[slot, o + BLK:o + 3 * BLK, :] = _normalize(_nt(e1, v_f[slot, b].astype(BF16)), l1)
        c = _normalize(_nt(e0, two_blocks(v_f, slot, b)), l0)
        ctx[slot, o:o + BLK, :] = c[:BLK]
        ctx[slot, o + 3 * BLK:o + SQ, :] = c[BLK:]

    def attend_own(slot):
        q = q_own[:, slot * 128:(slot + 1) * 128]
        s = [scores(slot, q, b) for b in range(B)]
        for b in range(B):
            context(slot, s[b], b)

    def attend(s, t):
        qs, wt = project(weights(WQ, s)), weights(WQ, t)
        s0, qt, s1 = scores(s, qs, 0), project(wt), scores(s, qs, 1)
        context(s, s0, 0)
        t0 = scores(t, qt, 0)
        context(s, s1, 1)
        t1 = scores(t, qt, 1)
        context(t, t0, 0)
        context(t, t1, 1)

    def accumulate(rows, c, o, first=False, last=False):
        cols = pl.ds(c * 128, 128)
        if not first:
            o = acc[rows, cols] + o
        if last:
            out[rows, cols] = o.astype(out.dtype)
        else:
            acc[rows, cols] = o

    def output(slots, col_tiles, headers=(None, None), split=1, **kw):
        w = {c: jnp.concatenate([weights(WO, s, c * 64, c * 64 + 64, h) for s, h in zip(slots, headers)], axis=0)
             for c in col_tiles}
        for i in range(split):
            rows = pl.ds(i * (T // split), T // split)
            lhs = jnp.concatenate([ctx[s, rows, :] for s in slots], axis=1)
            for c in col_tiles:
                accumulate(rows, c, _nn(lhs, pltpu.bitcast(w[c], BF16)), **kw)

    def wait_kv(*slots):
        for slot in slots:
            for cp in load_kvs[slot]:
                cp.wait()

    load_x.wait()
    x_b[...] = x_f[...].astype(BF16)
    q_own[...] = project(jnp.concatenate([weights(WQ, 0), weights(WQ, 1)], axis=1))

    load_wo.wait()
    bases = []
    for p in range(2):
        w = [wo_f[p * 128:(p + 1) * 128, c * 128:(c + 1) * 128] for c in range(4)]
        bases.append(_choose_base(jnp.concatenate(w, axis=0), 0))
        w = jnp.concatenate([_words(t) for t in w], axis=0)
        codes[WO, p] = _encode(w, bases[p])
        words[WO, p] = w
    plain[WO, 0], plain[WO, 1] = write_headers(WO, (0, 1), bases)
    for hop in o_first:
        hop.start()

    wait_kv(0)
    attend_own(0)
    wait_kv(1)
    attend_own(1)

    receive_headers(q_first)
    receive(q_first)
    for hop in (*q_far, *o_second):
        hop.start()
    output((0, 1), range(4), first=True)
    wait_kv(2, 5)
    receive_headers(q_second)
    attend(2, 5)

    receive(q_second)
    wait_kv(3, 4)
    receive_headers(o_first)
    attend(3, 4)

    receive(o_first)
    for hop in o_far:
        hop.start()
    receive_headers(q_far)
    output((2, 5), range(4))

    receive(q_far)
    wait_kv(6, 7)
    receive_headers(o_second)
    attend(6, 7)

    receive(o_second)
    receive_headers(o_far)
    output((3, 4), range(4))
    far = {slot: read_header(WO, slot) for slot in (6, 7)}
    mixed[0] = jnp.where(_first_head(T), ctx[6], ctx[7])
    mixed[1] = jnp.where(_first_head(T), ctx[7], ctx[6])

    @pl.when(functools.reduce(jnp.logical_or, [plain[hop.src] for hop in hops]))
    def _():
        for hop in hops:
            pl.when(plain[hop.src])(hop.words.wait_send)

    receive(o_far, 0)
    output((6, 7), (0, 1), (far[6], far[7]), last=True)
    receive(o_far, 1)
    output((6, 7), (2,), (far[6], far[7]), split=2, last=True)
    for i, (s, t) in enumerate(((6, 7), (7, 6))):
        if i == 1:
            for j, ref in enumerate((codes, heads)):
                sent = ref.at[:, pl.ds(0, 6)]
                pltpu.make_async_remote_copy(sent, sent, send_sem.at[j], recv_sem.at[0],
                                             device_id=(right,), device_id_type=MESH).wait_send()
        receive(o_far, 2 + i)
        w = jnp.concatenate([weights(WO, s, 192, 224, far[s]), weights(WO, t, 224, 256, far[t])], axis=0)
        for j in range(4):
            rows = pl.ds(j * (T // 4), T // 4)
            accumulate(rows, 3, _nn(mixed[i, rows, :], pltpu.bitcast(w, BF16)), last=i == 1)


def pallas_dist_sparse_attn_blocksparse_qseq_b2_sq256_skv256_hq4_dh64_kernel(
    x: jax.Array,
    Wq: jax.Array,
    K_ext: jax.Array,
    V_ext: jax.Array,
    Wo: jax.Array,
):
    kt = jnp.transpose(K_ext, (0, 2, 3, 1)).reshape(B, 16 * BLK, SKV)
    vt = jnp.transpose(V_ext, (0, 2, 3, 1)).reshape(B, 16 * BLK, SKV)
    out = pl.pallas_call(
        _kernel_body,
        out_shape=pltpu.VMEM((T, D), OUT_DTYPE),
        in_specs=[pl.BlockSpec(memory_space=pltpu.HBM)] * 5,
        out_specs=pl.BlockSpec(memory_space=pltpu.VMEM),
        scratch_shapes=[
            pltpu.VMEM((T, D), F32),
            pltpu.VMEM((2, D, 128), F32),
            pltpu.VMEM((256, D), F32),
            pltpu.VMEM((8, B, 128, SKV), F32),
            pltpu.VMEM((8, B, 128, SKV), F32),
            pltpu.VMEM((T, D), BF16),
            pltpu.VMEM((T, 256), F32),
            pltpu.VMEM((2, 8, WORDS, 128), I32),
            pltpu.VMEM((2, 8, CODES, 128), I32),
            pltpu.VMEM((2, 8, 2, 128), I32),
            pltpu.VMEM((8, T, 128), BF16),
            pltpu.VMEM((2, T, 128), BF16),
            pltpu.VMEM((T, D), F32),
            pltpu.SemaphoreType.DMA((18 + 2 * len(FIRST_SPANS),)),
            pltpu.SemaphoreType.DMA((14,)),
            pltpu.SemaphoreType.DMA((42,)),
            pltpu.SemaphoreType.REGULAR,
        ],
        compiler_params=pltpu.CompilerParams(
            collective_id=0,
            vmem_limit_bytes=48 * 2**20,
            disable_bounds_checks=True,
            disable_semaphore_checks=True,
        ),
    )(x.reshape(T, D), Wq, kt, vt, Wo)
    return out.reshape(B, SQ, D)
```
